```python
import numpy as np

kernel_name = "dist_matmul_relu_kshard_i_m1024_n1024_k512"

def setup_inputs():
    A = np.random.randn(1024, 2048).astype(np.float32)
    B = np.random.randn(2048, 1024).astype(np.float32)
    return {"A": A, "B": B}

def reference(A: np.ndarray, B: np.ndarray) -> np.ndarray:
    z = A @ B
    return np.maximum(z, 0.0)
```

```python
import functools
import jax
import jax.numpy as jnp
from jax import lax
from jax.experimental import pallas as pl
from jax.experimental.pallas import tpu as pltpu

M, N, K = 1024, 1024, 512
BLK = M // 4
Q = BLK // 4
F32, BF16 = jnp.float32, jnp.bfloat16
MESH = pl.DeviceIdType.MESH

def make(pieces=((0, 1, 0, 128), (1, 2, 0, 128), (0, 2, 128, 128), (0, 2, 256, 256), (0, 2, 512, 512)),
         bcols=((0, 128), (128, 128), (256, 256), (512, 512))):
  NP = len(pieces)

  def body(a_hbm, b_hbm, out, a32, b32, a16, b16, s1, r1, s2, r2, s3, r3, acc, lsem, ssem, rsem):
    me = lax.axis_index("i")
    yp, xp, dg = me ^ 1, 3 - me, me ^ 2
    nbr = (yp, xp)
    DG, YP, XP, ME = range(4)
    owner = (dg, yp, xp, me)

    nl = [0]
    def load(src, dst):
      c = pltpu.make_async_copy(src, dst, lsem.at[nl[0]]); nl[0] += 1
      c.start()
      return c
    def load_a(role, q0, nq):
      return load(a_hbm.at[pl.ds(owner[role] * BLK + q0 * Q, nq * Q)], a32.at[pl.ds(role * BLK + q0 * Q, nq * Q)])
    def load_b(c0, w):
      return load(b_hbm.at[:, pl.ds(c0, w)], b32.at[:, pl.ds(c0, w)])

    lb = {}
    lb[bcols[0]] = load_b(*bcols[0])
    la_d = [load_a(DG, 0, 2)]
    bar = pltpu.get_barrier_semaphore()
    for n in nbr:
      pl.semaphore_signal(bar, 1, device_id=(n,), device_id_type=MESH)
    la_d.append(load_a(DG, 2, 2))
    for bc in bcols[1:]:
      lb[bc] = load_b(*bc)
    la_y = load_a(YP, 0, 4)
    la_x = load_a(XP, 0, 4)
    la_m = load_a(ME, 0, 4)

    def cast_a(r0, nr):
      a16[pl.ds(r0, nr), :] = a32[pl.ds(r0, nr), :].astype(BF16)
    def cast_b(c0, w):
      b16[:, pl.ds(c0, w)] = b32[:, pl.ds(c0, w)].astype(BF16)

    ns = [0]
    sends = []
    def remote(src, dst, link):
      i = ns[0]; ns[0] += 1
      c = pltpu.make_async_remote_copy(src, dst, ssem.at[i], rsem.at[i], device_id=(nbr[link],), device_id_type=MESH)
      sends.append(c)
      return c

    got_a, got_b = set(), set()
    c1 = []
    for i, (q0, q1, c0, w) in enumerate(pieces):
      for s in range(q0, q1):
        if s not in got_a:
          got_a.add(s); la_d[s].wait(); cast_a(DG * BLK + s * 2 * Q, 2 * Q)
      for bc in bcols:
        if bc[0] < c0 + w and c0 < bc[0] + bc[1] and bc not in got_b:
          got_b.add(bc); lb[bc].wait(); cast_b(*bc)
      p = jnp.dot(a16[pl.ds(DG * BLK + q0 * 2 * Q, (q1 - q0) * 2 * Q), :], b16[:, pl.ds(c0, w)], preferred_element_type=F32).astype(BF16)
      for s in range(q0, q1):
        for h in range(2):
          s1[h, s, :, pl.ds(c0, w)] = p[((s - q0) * 2 + h) * Q:((s - q0) * 2 + h + 1) * Q]
      if i == 0:
        pl.semaphore_wait(bar, 2)
      for h in range(2):
        c = remote(s1.at[h, pl.ds(q0, q1 - q0), :, pl.ds(c0, w)], r1.at[h, pl.ds(q0, q1 - q0), :, pl.ds(c0, w)], h)
        c.start(); c1.append(c)

    def part(role, s, h):
      return jnp.dot(a16[pl.ds(role * BLK + (2 * s + h) * Q, Q), :], b16[...], preferred_element_type=F32)

    la_y.wait(); cast_a(YP * BLK, BLK)
    la_x.wait(); cast_a(XP * BLK, BLK)
    c2 = []
    for h, role in ((0, YP), (1, XP)):
      for s in range(2):
        s2[h, s] = part(role, s, h).astype(BF16)
      c = remote(s2.at[h], r2.at[h], h); c.start(); c2.append(c)

    la_m.wait(); cast_a(ME * BLK, BLK)
    for c in c1:
      c.wait_recv()
    c3 = [[None, None], [None, None]]
    for s in range(2):
      for link, role, h in ((0, YP, 1), (1, XP, 0)):
        s3[link, s] = (part(role, s, h) + r1[h, s].astype(F32)).astype(BF16)
        c = remote(s3.at[link, s], r3.at[link, s], link); c.start(); c3[link][s] = c

    for c in c2:
      c.wait_recv()
    for s in range(2):
      for h in range(2):
        acc[s, h] = part(ME, s, h) + r2[h, s].astype(F32)
    c4 = [[None, None], [None, None]]
    for s in range(2):
      for h in range(2):
        c3[1 - h][s].wait_recv()
        z = acc[s, h] + r3[1 - h, s].astype(F32)
        out[pl.ds(pl.multiple_of(me * BLK + (2 * s + h) * Q, Q), Q), :] = jnp.maximum(z, 0.0).astype(BF16)
      rows = out.at[pl.ds(pl.multiple_of(me * BLK + 2 * s * Q, 2 * Q), 2 * Q)]
      for link in range(2):
        c = remote(rows, rows, link); c.start(); c4[link][s] = c

    c6 = []
    for s in range(2):
      for link in range(2):
        c4[1 - link][s].wait_recv()
        rows = out.at[pl.ds(pl.multiple_of(nbr[1 - link] * BLK + (2 * s + link) * Q, Q), Q)]
        c = remote(rows, rows, link); c.start(); c6.append(c)
    for c in sends:
      c.wait_send()
    for c in c6:
      c.wait_recv()

  nrem = 2 * NP + 2 + 4 + 4 + 4
  def f(A, B):
    return pl.pallas_call(
        body,
        out_shape=jax.ShapeDtypeStruct((M, N), BF16),
        in_specs=[pl.BlockSpec(memory_space=pltpu.HBM)] * 2,
        out_specs=pl.BlockSpec(memory_space=pltpu.VMEM),
        scratch_shapes=[
            pltpu.VMEM((M, K), F32), pltpu.VMEM((K, N), F32), pltpu.VMEM((M, K), BF16), pltpu.VMEM((K, N), BF16),
            pltpu.VMEM((2, 2, Q, N), BF16), pltpu.VMEM((2, 2, Q, N), BF16),
            pltpu.VMEM((2, 2, Q, N), BF16), pltpu.VMEM((2, 2, Q, N), BF16),
            pltpu.VMEM((2, 2, Q, N), BF16), pltpu.VMEM((2, 2, Q, N), BF16),
            pltpu.VMEM((2, 2, Q, N), F32),
            pltpu.SemaphoreType.DMA((5 + len(bcols),)), pltpu.SemaphoreType.DMA((nrem,)), pltpu.SemaphoreType.DMA((nrem,)),
        ],
        compiler_params=pltpu.CompilerParams(collective_id=0, vmem_limit_bytes=48 * 2**20),
    )(A, B)
  return f


_kernel = make()


def pallas_dist_matmul_relu_kshard_i_m1024_n1024_k512_kernel(A: jax.Array, B: jax.Array):
  return _kernel(A, B)
```

```python
import contextlib
import functools
import jax
import jax.numpy as jnp
from jax import lax
from jax.experimental import pallas as pl
from jax.experimental.pallas import tpu as pltpu

M, N, K = 1024, 1024, 512
BLK = M // 4
G = BLK // 2
Q = BLK // 4
F32, BF16, I32 = jnp.float32, jnp.bfloat16, jnp.int32
MESH = pl.DeviceIdType.MESH
DG, YP, XP, ME = range(4)

W = 64
CW = 44
BASE = CW + 2
OV = W - CW
HI, SIGNS, ONES = -0x10000, -0x7FFF8000, 0x00010001
srl = lax.shift_right_logical


def pack_lo(a, b):
  return pltpu.bitcast(pltpu.pack_elementwise([a, b], packed_dtype=jnp.int16), I32)


def compress(word, tmp, dst):
  cnt = jnp.zeros((8, 128), I32)
  stay = [[{}, {}, {}], [{}, {}, {}]]
  def push(h, k, i, x):
    if k == 3:
      tmp[h, i] = x
      return
    s = 1 << k
    if i < s:
      stay[h][k][i] = x
      return
    m = (x & s) != 0
    stay[h][k][i] = jnp.where(m, 0, x)
    push(h, k + 1, i - s, jnp.where(m, x, stay[h][k].pop(i - s)))
  for i in range(W):
    w = word(i)
    t = (w + 0x7FFF7FFF) & SIGNS
    d = i * ONES - cnt
    cnt = cnt + srl(t, 15)
    tmp[2, i] = t
    push(0, 0, i, pack_lo(d, w))
    push(1, 0, i, (w & HI) | srl(d, 16))
  for h in range(2):
    for k in range(3):
      for i in sorted(stay[h][k]):
        push(h, k + 1, i, stay[h][k].pop(i))
  over = jnp.max((cnt & 0xFFFF) + srl(cnt, 16)) > 2 * CW
  keep = jnp.where(over, 0, -1)
  pk = lambda a, b: srl(a, 16) | (b & HI)
  for r in range(4):
    x = {}
    for h in range(2):
      for rho in (r, 7 - r):
        v = [tmp[h, rho + 8 * j] for j in range(8)]
        for s in (1, 2, 4):
          m = [None] * s + [(v[j] & (8 * s)) != 0 for j in range(s, 8)]
          st = [v[j] if m[j] is None else jnp.where(m[j], 0, v[j]) for j in range(8)]
          v = [jnp.where(m[j + s], v[j + s], st[j]) if j + s < 8 else st[j] for j in range(8)]
        for j in range(8):
          x[h, rho + 8 * j] = v[j]
    for rho in (r, 7 - r):
      for j in range(rho, W, 8):
        a, b = x[0, j], x[1, j]
        if j >= CW:
          dst[2 + j] = pk(a, b)
          continue
        o = 2 * CW - 1 - j
        if o < W:
          a = a | (x[1, o] & keep); b = b | (x[0, o] & keep)
        dst[2 + j] = pk(a, b) | tmp[2, j]
  orr = lambda a, b: a | b
  dst[0] = functools.reduce(orr, [srl(tmp[2, CW + k], k) for k in range(16)])
  dst[1] = functools.reduce(orr, [srl(tmp[2, CW + 16 + k], k) for k in range(OV - 16)]) | over.astype(I32)
  return over


def decompress(src, over, tmp, put):
  f0, f1 = src[0], src[1]
  def flags(q):
    if q < CW:
      return src[2 + q] & SIGNS
    f, k = (f0, q - CW) if q - CW < 16 else (f1, q - CW - 16)
    return (f << k if k else f) & SIGNS
  def val(h, q):
    if q < CW:
      w = src[2 + q]
      return srl(w, 16) if h else w
    e, c = src[2 + q], src[2 + 2 * CW - 1 - q]
    return jnp.where(over, srl(e, 16), c) if h else jnp.where(over, e, srl(c, 16))
  cnt = jnp.zeros((8, 128), I32)
  for q in range(W):
    if q >= 8:
      tmp[2, q] = q * ONES - cnt
    if q < W - 1:
      cnt = cnt + srl(flags(q), 15)
  for rho in range(8):
    d = [None] + [tmp[2, rho + 8 * j] for j in range(1, 8)]
    for h in range(2):
      v = [val(h, rho + 8 * j) for j in range(8)]
      for s in (4, 2, 1):
        v = [v[j] if j < s else jnp.where((d[j] & ((8 * s) << (16 * h))) != 0, v[j - s], v[j]) for j in range(8)]
      for j in range(1, 8):
        tmp[h, rho + 8 * j] = v[j]
  cnt = jnp.zeros((8, 128), I32)
  win = [[{}, {}, {}], [{}, {}, {}]]
  for q in range(W):
    t = flags(q)
    g = srl(t, 15)
    d = q * ONES - cnt
    cnt = cnt + g
    r = []
    for h in range(2):
      x = val(h, q) if q < 8 else tmp[h, q]
      for k in (2, 1, 0):
        s = 1 << k
        win[h][k][q] = x
        if q >= s:
          x = jnp.where((d & (s << (16 * h))) != 0, win[h][k].pop(q - s), x)
      r.append(x)
    put(q, pack_lo(r[0], r[1]) & (t - g))


DEFAULT = (("b", 0, 128), ("a", 0), ("p", 0, 1, 0, 128), ("a", 1), ("p", 1, 2, 0, 128),
           ("b", 128, 128), ("p", 0, 2, 128, 128), ("b", 256, 128), ("p", 0, 2, 256, 128),
           ("b", 384, 256), ("p", 0, 2, 384, 256), ("b", 640, 384), ("p", 0, 2, 640, 384))


def make(scopes=False, plan=DEFAULT, cp={}, refcast=True):
  sc = (lambda n: jax.named_scope(n)) if scopes else (lambda n: contextlib.nullcontext())
  nload = sum(p[0] != "p" for p in plan) + 2
  HALF = BASE // 2

  def body(a_hbm, b_hbm, out, a32, b32, a16, b16, s1, r1, s2, r2, s3, r3, acc, cbuf, tmp, ssem, osem, fsem):
    me = lax.axis_index("i")
    yp, xp, dg = me ^ 1, 3 - me, me ^ 2
    nbr = (yp, xp)
    owner = (dg, yp, xp, me)
    sends = []

    def rcopy(src, dst, send_sem, recv_sem, dev):
      return pltpu.make_async_remote_copy(src, dst, send_sem, recv_sem, device_id=(dev,), device_id_type=MESH)

    def remote(refs, link, rsem):
      rcopy(*refs(), ssem, rsem, nbr[link]).start()
      sends.append(refs)

    def wait_recv(rsem, ref):
      pltpu.make_async_copy(ref, ref, rsem).wait()

    def cast_a(r0, nr):
      a16[pl.ds(r0, nr), :] = a32[pl.ds(r0, nr), :].astype(BF16)
    def cast_b(c0, w):
      b16[:, pl.ds(c0, w)] = b32[:, pl.ds(c0, w)].astype(BF16)
    def part(role, s, h):
      return jnp.dot(a16[pl.ds(role * BLK + s * G + h * Q, Q), :], b16[...], preferred_element_type=F32)
    def half(h):
      return pl.ds(h * Q, Q)
    def words(role, s, part):
      return cbuf.at[role, s, pl.ds(part * HALF, HALF)]
    def spill(role, s, part=None):
      return cbuf.at[role, s, pl.ds(BASE, OV) if part is None else pl.ds(BASE + part * (OV // 2), OV // 2)]
    def flagged(role, s):
      return (cbuf[role, s, 1][0, 0] & 1) != 0
    def expand(role, s, chip, over):
      if refcast:
        oi = out.bitcast(I32)
        r0 = pl.multiple_of(chip * (BLK // 2) + s * (G // 2), G // 2)
        def put(q, w):
          oi[pl.ds(r0 + 8 * (q // 8), 8), pl.ds(128 * (q % 8), 128)] = w
      else:
        r0 = pl.multiple_of(chip * BLK + s * G, G)
        def put(q, w):
          out[pl.ds(r0 + 16 * (q // 8), 16), pl.ds(128 * (q % 8), 128)] = pltpu.bitcast(w, BF16)
      decompress(cbuf.at[role, s], over, tmp, put)

    @functools.partial(pl.run_scoped, lsem=pltpu.SemaphoreType.DMA((nload,)), rsem=pltpu.SemaphoreType.DMA((8,)),
                       esem=pltpu.SemaphoreType.DMA((3, 2)))
    def _(lsem, rsem, esem):
      R1, R2, R3, G0, G1F, G1R, D0 = 0, 1, 2, 4, 5, 6, 7
      nl = [0]
      def load(src, dst):
        c = pltpu.make_async_copy(src, dst, lsem.at[nl[0]]); nl[0] += 1
        c.start()
        return c
      def load_a(role, r0, nr):
        return load(a_hbm.at[pl.ds(owner[role] * BLK + r0, nr)], a32.at[pl.ds(role * BLK + r0, nr)])
      loads = {}
      bar = pltpu.get_barrier_semaphore()
      for i, p in enumerate(plan):
        if p[0] == "a":
          loads[i] = load_a(DG, G * p[1], G)
        elif p[0] == "b":
          loads[i] = load(b_hbm.at[:, pl.ds(p[1], p[2])], b32.at[:, pl.ds(p[1], p[2])])
        if i == 1:
          for n in nbr:
            pl.semaphore_signal(bar, 1, device_id=(n,), device_id_type=MESH)
      yx = a32.at[pl.ds(YP * BLK, 2 * BLK)]
      for role in (YP, XP):
        pltpu.make_async_copy(a_hbm.at[pl.ds(owner[role] * BLK, BLK)], a32.at[pl.ds(role * BLK, BLK)], lsem.at[nl[0]]).start()
      la_yx = pltpu.make_async_copy(yx, yx, lsem.at[nl[0]]); nl[0] += 1
      la_m = load_a(ME, 0, BLK)

      first = True
      for i, p in enumerate(plan):
        if p[0] == "a":
          with sc(f"wa{p[1]}"): loads[i].wait()
          cast_a(DG * BLK + p[1] * G, G)
        elif p[0] == "b":
          with sc(f"wb{p[1]}"): loads[i].wait()
          cast_b(p[1], p[2])
        else:
          _, q0, q1, c0, w = p
          v = jnp.dot(a16[pl.ds(DG * BLK + q0 * G, (q1 - q0) * G), :], b16[:, pl.ds(c0, w)], preferred_element_type=F32).astype(BF16)
          for s in range(q0, q1):
            s1[s, :, pl.ds(c0, w)] = v[(s - q0) * G:(s - q0 + 1) * G]
          if first:
            with sc("bar"): pl.semaphore_wait(bar, 2)
            first = False
          with sc(f"s1_{i}"):
            for h in range(2):
              remote(lambda h=h, q0=q0, q1=q1, c0=c0, w=w: tuple(r.at[pl.ds(q0, q1 - q0), half(h), pl.ds(c0, w)] for r in (s1, r1)), h, rsem.at[R1])

      with sc("wyx"): la_yx.wait()
      cast_a(YP * BLK, 2 * BLK)
      for h, role in ((0, YP), (1, XP)):
        for s in range(2):
          s2[s, half(h)] = part(role, s, h).astype(BF16)
        with sc(f"s2_{h}"): remote(lambda h=h: (s2.at[:, half(h)], r2.at[:, half(h)]), h, rsem.at[R2])
      la_m.wait(); cast_a(ME * BLK, BLK)

      with sc("w1"): wait_recv(rsem.at[R1], r1)
      for s in range(2):
        for link, role, h in ((0, YP, 1), (1, XP, 0)):
          s3[s, half(h)] = (part(role, s, h) + r1[s, half(h)].astype(F32)).astype(BF16)
          with sc(f"s3_{link}{s}"): remote(lambda h=h, s=s: (s3.at[s, half(h)], r3.at[s, half(h)]), link, rsem.at[R3 + s])

      with sc("w2"): wait_recv(rsem.at[R2], r2)
      for s in range(2):
        for h in range(2):
          acc[s, half(h)] = part(ME, s, h) + r2[s, half(h)].astype(F32)

      @pl.loop(0, 2)
      def _(s):
        with sc("w3"): wait_recv(rsem.at[R3 + s], r3.at[s])
        r0 = pl.multiple_of(me * BLK + s * G, G)
        cache = {}
        def word(i):
          if i % 8 == 0:
            rows = pl.ds(2 * i, 16)
            z = jnp.maximum(acc[s, rows] + r3[s, rows].astype(F32), 0.0)
            out[pl.ds(r0 + 2 * i, 16), :] = z.astype(BF16)
            cache[0] = z
          return pltpu.bitcast(cache[0][:, 128 * (i % 8):128 * (i % 8 + 1)].astype(BF16), I32) & 0x7FFF7FFF
        over = compress(word, tmp, cbuf.at[ME, s])
        with sc("s4"):
          for first in (True, False):
            for link in range(2):
              p = 1 - link if first else link
              sem = rsem.at[jnp.where(s == 0, G0, G1F if first else G1R)]
              rcopy(words(ME, s, p), words(YP + link, s, p), ssem, sem, nbr[link]).start()
        @pl.when(over)
        def _():
          for link in range(2):
            c = rcopy(spill(ME, s), spill(YP + link, s), osem.at[link], esem.at[YP + link, s], nbr[link])
            c.start()
            c.wait_send()

      @pl.loop(0, 5)
      def _(i):
        s = jnp.where(i < 4, i // 2, 0)
        role = jnp.where(i < 4, YP + i % 2, DG)
        @pl.when((i == 0) | (i == 2))
        def _():
          with sc("w4"):
            @pl.when(i == 0)
            def _():
              wait_recv(rsem.at[G0], cbuf.at[pl.ds(YP, 2), 0, pl.ds(0, BASE)])
            @pl.when(i == 2)
            def _():
              wait_recv(rsem.at[G1F], cbuf.at[pl.ds(YP, 2), 1, pl.ds(0, HALF)])
          for link in range(2):
            @pl.when(i == 0)
            def _():
              rcopy(words(XP - link, 0, link), words(DG, 0, link), ssem, rsem.at[D0], nbr[link]).start()
            @pl.when(i == 2)
            def _():
              rcopy(words(XP - link, 1, link), words(DG, 1, link), ssem, fsem.at[0], nbr[link]).start()
          @pl.when(i == 2)
          def _():
            with sc("w5"): wait_recv(rsem.at[G1R], cbuf.at[pl.ds(YP, 2), 1, pl.ds(0, HALF)])
        @pl.when(i == 4)
        def _():
          with sc("w6"): wait_recv(rsem.at[D0], cbuf.at[DG, 0, pl.ds(0, BASE)])
        over = flagged(role, s)
        @pl.when(over)
        def _():
          wait_recv(esem.at[role, s], spill(role, s))
          @pl.when(i < 4)
          def _():
            link = XP - role
            dev = jnp.where(link == 0, yp, xp)
            @pl.when(s == 0)
            def _():
              rcopy(spill(role, s, link), spill(DG, s, link), osem.at[0], esem.at[DG, 0], dev).start()
            @pl.when(s == 1)
            def _():
              rcopy(spill(role, s, link), spill(DG, s, link), osem.at[0], fsem.at[1], dev).start()
            rcopy(spill(role, s, link), spill(DG, s, link), osem.at[0], fsem.at[1], dev).wait_send()
        chip = jnp.where(role == YP, yp, jnp.where(role == XP, xp, dg))
        with sc("dec"): expand(role, s, chip, over)

    with sc("wsend"):
      for refs in sends:
        rcopy(*refs(), ssem, fsem.at[0], me).wait_send()
      for _ in range(12):
        rcopy(words(ME, 0, 0), words(ME, 0, 0), ssem, fsem.at[0], me).wait_send()
    with sc("w7"): wait_recv(fsem.at[0], cbuf.at[DG, 1, pl.ds(0, BASE)])
    over = flagged(DG, 1)
    @pl.when(over)
    def _():
      wait_recv(fsem.at[1], spill(DG, 1))
    with sc("dec"): expand(DG, 1, dg, over)

  def f(A, B):
    grp = pltpu.VMEM((2, G, N), BF16)
    return pl.pallas_call(
        body,
        out_shape=jax.ShapeDtypeStruct((M, N), BF16),
        in_specs=[pl.BlockSpec(memory_space=pltpu.HBM)] * 2,
        out_specs=pl.BlockSpec(memory_space=pltpu.VMEM),
        scratch_shapes=[
            pltpu.VMEM((M, K), F32), pltpu.VMEM((K, N), F32), pltpu.VMEM((M, K), BF16), pltpu.VMEM((K, N), BF16),
            grp, grp, grp, grp, grp, grp,
            pltpu.VMEM((2, G, N), F32),
            pltpu.VMEM((4, 2, 2 + W, 8, 128), I32), pltpu.VMEM((3, W, 8, 128), I32),
            pltpu.SemaphoreType.DMA, pltpu.SemaphoreType.DMA((2,)), pltpu.SemaphoreType.DMA((2,)),
        ],
        compiler_params=pltpu.CompilerParams(collective_id=0, vmem_limit_bytes=48 * 2**20, **cp),
    )(A, B)
  return f


_kernel = make()


def pallas_dist_matmul_relu_kshard_i_m1024_n1024_k512_kernel(A: jax.Array, B: jax.Array):
  return _kernel(A, B)
```

```python
import functools
import jax, jax.numpy as jnp
from jax import lax
from jax.experimental import pallas as pl
from jax.experimental.pallas import tpu as pltpu
F32, BF16, I32 = jnp.float32, jnp.bfloat16, jnp.int32

HI, SIGNS, ONES = -0x10000, -0x7FFF8000, 0x00010001
WIDE, MID, GAP, LOW = 0x70007000, 0x08000800, 0x78007800, 0x07FF07FF
TOP = -0x80000000
srl = lax.shift_right_logical
VREG = (8, 128)


def shift(x, n):
  return x << n if n > 0 else srl(x, -n) if n < 0 else x

def or_all(xs):
  return functools.reduce(lambda a, b: a | b, xs)

def pack_lo(a, b):
  return pltpu.bitcast(pltpu.pack_elementwise([a, b], packed_dtype=jnp.int16), I32)

def to_word(a, b):
  return pltpu.bitcast(pltpu.pack_elementwise([a, b], packed_dtype=BF16), I32)

def from_word(w):
  return pltpu.bitcast(w << 16, F32), pltpu.bitcast(w & HI, F32)

def gap_words(ws):
  return [or_all([srl(w & GAP, 11 - 4 * j) if j < 3 else (w & GAP) << 1 for j, w in enumerate(ws[k:k + 4])]) for k in range(0, len(ws), 4)]

def gap_len(n):
  return -(-n // 4)

def mid_planes(ws):
  return [or_all([shift(w & MID, j - 11) for j, w in enumerate(ws[k:k + 16])]) for k in range(0, len(ws), 16)]

def mid_bit(planes, i):
  return shift(planes[i // 16], 11 - i % 16) & MID

def gap_bits(ref, at, i):
  return shift(ref[at + i // 4], 11 - 4 * (i % 4)) & GAP

def dense_len(n):
  return 1 + 3 * n // 4

def dense_encode(ws, mx, dst, at):
  x = 3 * len(ws) // 4
  b = (srl(to_word(mx, mx), 7) - 31) & 0xFF
  base = b * (ONES << 7)
  ws = [w - base for w in ws]
  left = or_all(ws) & WIDE
  head = b
  for k, z in enumerate(mid_planes(ws)):
    z = ~z
    for e in range(2):
      low = z & -z
      head = head | (lax.clz(low) << (8 + 12 * k + 6 * e))
      z = z ^ low
    left = left | z
  dst[at] = head | jnp.where(left != 0, 63 << 8, 0)
  for d, w in enumerate(ws[x:]):
    w = (w & LOW) | (srl(w, 4) & MID)
    for i in range(3):
      dst[at + 1 + 3 * d + i] = (ws[3 * d + i] & ~GAP) | ((w << (11 - 4 * i)) & GAP)
  return ws, jnp.where(left != 0, 1.0, 0.0)

def dense_wide(src):
  return jnp.max(jnp.where((src[0] & (63 << 8)) == 63 << 8, 1.0, 0.0)) > 0

def dense_planes(src, n):
  planes = []
  for k in range(n // 16):
    at = [srl(src[0], 8 + 12 * k + 6 * e) for e in range(2)]
    planes.append(~or_all([srl(jnp.where((a & 32) != 0, 0, TOP), a & 31) for a in at]))
  return planes

def dense_decode(src, n, dst, to):
  x = 3 * n // 4
  base = (src[0] & 0xFF) * (ONES << 7)
  planes = dense_planes(src, n)
  msg = [src[1 + i] for i in range(x)]
  ws = [w & ~GAP for w in msg]
  for d in range(n - x):
    w = or_all([srl(msg[3 * d + i] & GAP, 11 - 4 * i) for i in range(3)])
    ws.append((w & LOW) | ((w & MID) << 4))
  for i, w in enumerate(ws):
    dst[to + i] = (w | mid_bit(planes, i)) + base

def dense_repair(src, n, gaps, dst, to):
  planes = dense_planes(src, n)
  for i in range(n):
    dst[to + i] = dst[to + i] - mid_bit(planes, i) + gap_bits(gaps, 0, i)

W = 64
C = 82
NV = C // 2
MSG = 33
REST = 24
EXTRA = REST + gap_len(NV) + 1
T_W, T_T, T_D, T_X = 0, W, 2 * W, 3 * W
TMP = 5 * W

PAIRS = ((0, 3), (1, 2), (4, 7), (5, 6))
META = NV
LATE_AT = list(range(13, 16)) + list(range(29, 33))
EARLY_AT = [i for i in range(MSG) if i not in LATE_AT]
FLAG_AT = EARLY_AT[:4]
EARLY_V = [5 * r + i for pair in PAIRS[:3] for r in pair for i in range(5)] + [NV - 1, META]
LATE_V = [5 * r + i for r in PAIRS[3] for i in range(5)]
HOME = dict(list(zip(EARLY_V[:22], EARLY_AT[4:])) + list(zip(LATE_V[:7], LATE_AT)))
def _cut(vs, ats):
  n = len(vs)
  return {v: [(ats[2 * k], 11, ~LOW), (ats[2 * k + 1], 6, ~LOW), (ats[2 * n + k // 5], 1 + k % 5, shift_const(MID, k % 5))] for k, v in enumerate(vs)}
def shift_const(c, n):
  c = (c << n) & 0xFFFFFFFF
  return c - (1 << 32) if c >> 31 else c
CUT = {**_cut(EARLY_V[22:], EARLY_AT[4:]), **_cut(LATE_V[7:], LATE_AT)}

def partner(x):
  return pltpu.roll(x, 4, 0)

def pair_total(cnt):
  n = (cnt & 0xFFFF) + srl(cnt, 16)
  return n + partner(n)

def slot_at(j):
  return (NV - 1, j % 2) if j >= 80 else (5 * (j % 8) + j // 16, (j // 8) % 2)

def rest_at(p):
  m = p // 8 - (11 if p % 8 < 2 else 10)
  return 3 * (p % 8) + m // 2, m % 2

def sparse_encode(word, tmp, dst, put):
  cnt = jnp.zeros(VREG, I32)
  mx = jnp.zeros(VREG, I32)
  for q in range(W):
    w = word(q) & ~SIGNS
    put(q, w)
    mx = jnp.maximum(mx, jnp.maximum(w, w << 16))
    t = (w + ~SIGNS) & SIGNS
    tmp[T_W + q] = w
    tmp[T_T + q] = t
    tmp[T_D + q] = q * ONES - cnt
    cnt = cnt + srl(t, 15)
  for k, at in enumerate(FLAG_AT):
    dst[at] = or_all([shift(tmp[T_T + 16 * k + j], -j) for j in range(16)])
  z_lo = W - (cnt & 0xFFFF)
  mx = jnp.maximum(mx, partner(mx))
  b = (srl(mx, 23) - 31) & 0xFF
  base = b * (ONES << 7)

  stay = [{}, {}, {}]
  def push(k, i, x):
    if k == 3:
      tmp[T_X + i] = x
      return
    s = 1 << k
    if i < s:
      stay[k][i] = x
      return
    m = (x & s) != 0
    stay[k][i] = jnp.where(m, 0, x)
    push(k + 1, i - s, jnp.where(m, x, stay[k].pop(i - s)))
  seen = tiny = jnp.zeros(VREG, I32)
  for q in range(W):
    t = tmp[T_T + q]
    w = (((tmp[T_W + q] | SIGNS) - base) ^ MID) & (t - srl(t, 15))
    tmp[T_W + q] = w
    seen = seen | w
    tiny = tiny + srl(w & MID, 11)
    push(0, q, pack_lo(tmp[T_D + q], w))
  full = pair_total(cnt) > 2 * C
  more = full | (pair_total(tiny) > 2) | ((seen & WIDE) != 0)
  more = jnp.max(jnp.max(jnp.where(more, 1.0, 0.0), axis=1, keepdims=True), axis=0, keepdims=True)
  for q in range(W):
    push(0, W + q, (tmp[T_W + q] & HI) | (srl(tmp[T_D + q], 16) + z_lo))
  for k in range(3):
    for i in sorted(stay[k]):
      push(k + 1, i, stay[k].pop(i))
  keep = jnp.where(full, 0, -1)

  pack = lambda a, b: srl(a, 16) | (b & HI)
  last = {}
  for pair in PAIRS:
    x = {}
    for r in pair:
      v = [tmp[T_X + r + 8 * m] for m in range(16)]
      for s in (1, 2, 4, 8):
        mv = [None] * s + [(v[m] & (8 * s)) != 0 for m in range(s, 16)]
        st = [v[m] if mv[m] is None else jnp.where(mv[m], 0, v[m]) for m in range(16)]
        v = [jnp.where(mv[m + s], v[m + s], st[m]) if m + s < 16 else st[m] for m in range(16)]
      for m in range(16):
        x[r + 8 * m] = v[m]
    for r in pair:
      def slot(j):
        o = 2 * C - 1 - j
        return x[j] | (partner(x[o]) & keep) if o < 2 * W else x[j]
      for i in range(5):
        tmp[T_W + 5 * r + i] = pack(slot(r + 16 * i), slot(r + 16 * i + 8))
      p0 = r + (88 if r < 2 else 80)
      for i in range(3):
        p = p0 + 16 * i
        dst[MSG + 3 * r + i] = pack(x[p], x[p + 8]) if p + 8 < 2 * W else srl(x[p], 16)
      if r < 2:
        last[r] = slot(80 + r)
  tmp[T_W + NV - 1] = pack(last[0], last[1])
  z = mid_planes([tmp[T_W + i] for i in range(NV)])
  small = []
  for e in range(2):
    m0, m01 = z[0] != 0, (z[0] | z[1]) != 0
    cur = jnp.where(m0, z[0], jnp.where(m01, z[1], z[2]))
    low = cur & -cur
    small.append(lax.clz(low) + jnp.where(m0, 0, jnp.where(m01, 32, 64)))
    z = [z[0] ^ jnp.where(m0, low, 0), z[1] ^ jnp.where(m0, 0, jnp.where(m01, low, 0)), z[2] ^ jnp.where(m01, 0, low)]
  more = jnp.where(jnp.broadcast_to(more, VREG) > 0, 127, 0)
  meta = b | ((small[0] | more) << 8) | (small[1] << 15)
  tmp[T_W + META] = (meta & 0x7FF) | (srl(meta, 11) << 16)
  parts = {}
  for v, pieces in CUT.items():
    for at, sh, mask in pieces:
      parts.setdefault(at, []).append((tmp[T_W + v] << sh) & mask)
  for v, at in HOME.items():
    dst[at] = or_all([tmp[T_W + v] & LOW] + parts[at])
  return more[0, 0] > 0

def sparse_gaps(tmp, dst):
  for k, g in enumerate(gap_words([tmp[T_W + i] for i in range(NV)])):
    dst[MSG + REST + k] = g
  dst[MSG + EXTRA - 1] = jnp.zeros(VREG, I32)

def gather(src, v):
  return or_all([srl(src[at] & mask, sh) for at, sh, mask in CUT[v]])

def sparse_decode(src, tmp, put, wait_extra, wait_late):
  w = gather(src, META)
  meta = (w & 0x7FF) | (srl(w, 16) << 11)
  small = [srl(meta, 8) & 127, srl(meta, 15)]
  any_more = small[0][0, 0] == 127
  cnt = jnp.zeros(VREG, I32)
  for q in range(W):
    t = shift(src[FLAG_AT[q // 16]], q % 16) & SIGNS
    g = srl(t, 15)
    tmp[T_T + q] = t - g
    tmp[T_D + q] = q * ONES - cnt
    cnt = cnt + g
  wait_extra(any_more)
  more, full = small[0] == 127, pair_total(cnt) > 2 * C
  z_lo = (W - (cnt & 0xFFFF)) << 16
  base = (meta & 0xFF) * (ONES << 7)
  planes = [or_all([srl(jnp.where(srl(a, 5) == k, TOP, 0), a & 31) for a in small]) for k in range(3)]
  def unpack(vs):
    for v in vs:
      w = gather(src, v) if v in CUT else src[HOME[v]] & LOW
      tmp[T_W + v] = w | jnp.where(more, gap_bits(src, MSG + REST, v), mid_bit(planes, v))
  unpack(EARLY_V[:-1])
  def dist(p):
    return (tmp[T_D + p], 0) if p < W else (tmp[T_D + p - W] + z_lo, 16)
  def half(w, h):
    return srl(w, 16) if h else w
  def start(p):
    if p < C:
      i, h = slot_at(p)
      return half(tmp[T_W + i], h)
    i, h = slot_at(2 * C - 1 - p)
    j, k = rest_at(p)
    return jnp.where(full, half(src[MSG + j], k), half(partner(tmp[T_W + i]), h))
  for pair in PAIRS:
    if pair == PAIRS[-1]:
      wait_late()
      unpack(LATE_V)
    for r in pair:
      v = [start(r + 8 * m) for m in range(16)]
      d = [None] + [dist(r + 8 * m) for m in range(1, 16)]
      for s in (8, 4, 2, 1):
        v = [v[m] if m < s else jnp.where((d[m][0] & ((8 * s) << d[m][1])) != 0, v[m - s], v[m]) for m in range(16)]
      for m in range(16):
        tmp[T_X + r + 8 * m] = v[m]
  win = [[{}, {}, {}], [{}, {}, {}]]
  def finish(h, p):
    x = tmp[T_X + p]
    d, off = dist(p)
    for k in (2, 1, 0):
      s = 1 << k
      win[h][k][p] = x
      if p - s in win[h][k]:
        x = jnp.where((d & (s << off)) != 0, win[h][k].pop(p - s), x)
    return x
  for p in range(W - 7, W):
    finish(1, p)
  for q in range(W):
    put(q, ((pack_lo(finish(0, q), finish(1, W + q)) ^ MID) + base) & tmp[T_T + q])


import contextlib

M, N, K = 1024, 1024, 512
BLK = M // 4
G = BLK // 2
Q = G // 2
MESH = pl.DeviceIdType.MESH
DG, YP, XP, ME = range(4)
U = Q * N // 2048

DEFAULT = (("b", 0, 128), ("a", 0), ("p", 0, 1, 0, 128, 0), ("a", 1), ("p", 1, 2, 0, 128, 0),
           ("b", 128, 128), ("p", 0, 1, 128, 128, 0), ("p", 1, 2, 128, 128, 0), ("b", 256, 128), ("p", 0, 2, 256, 128, 0),
           ("b", 384, 128), ("p", 0, 2, 384, 128, 0),
           ("b", 512, 256), ("p", 0, 2, 512, 256, 1), ("b", 768, 256), ("p", 0, 2, 768, 256, 1))


def make(scopes=False, plan=DEFAULT, cp={}):
  sc = (lambda n: jax.named_scope(n)) if scopes else (lambda n: contextlib.nullcontext())
  nload = sum(p[0] != "p" for p in plan) + 5
  SPLIT = (0, 16, MSG)
  layout, where, at, to, at_gap = [], {}, 0, 0, 0
  for p in plan:
    if p[0] == "p":
      _, s0, s1_, c0, w, packed = p
      n = (s1_ - s0) * (Q // 16) * (w // 128)
      ln = dense_len(n) if packed else n
      i = 0
      for s in range(s0, s1_):
        for r in range(Q // 16):
          for c in range(c0 // 128, (c0 + w) // 128):
            where[s, r, c] = (packed, (to if packed else at) + i); i += 1
      layout.append((n, ln, at, to, at_gap))
      at += ln
      if packed:
        to += n; at_gap += gap_len(n)
  LEN1, DEC1, GAP1 = at, max(to, 1), max(at_gap, 1)
  NP = len(layout)
  LU, GU = dense_len(U), gap_len(U)
  NFLAG = 2 * sum(lay[0] != lay[1] for lay in layout) + 8 + 2 + 5

  def body(a_hbm, b_hbm, out, a32, b32, a16, b16, s1, r1, g1, plain, su, ru, gu, kept, acc, zbuf, cbuf, tmp, flags, fsem):
    me = lax.axis_index("i")
    yp, xp, dg = me ^ 1, 3 - me, me ^ 2
    nbr = (yp, xp)
    owner = (dg, yp, xp, me)
    sends, maybe, sems = [], [], {}
    out_words = out.bitcast(I32)

    def rcopy(src, dst, send_sem, recv_sem, dev):
      return pltpu.make_async_remote_copy(src, dst, send_sem, recv_sem, device_id=(dev,), device_id_type=MESH)

    def remote(refs, link, rsem):
      rcopy(*refs(), sems['s'], rsem, nbr[link]).start()
      sends.append(refs)

    def send_gaps(jobs):
      @pl.when(jnp.max(functools.reduce(jnp.maximum, [job[0] for job in jobs])) > 0)
      def _():
        for j, (wide, at, n, refs, link, rsem) in enumerate(jobs):
          cond = jnp.max(wide) > 0
          flags[len(maybe) + j] = cond.astype(I32)
          @pl.when(cond)
          def _():
            src, dst = refs()
            for k, g in enumerate(gap_words([kept[at + i] for i in range(n)])):
              src[k] = g
            rcopy(src, dst, sems['o'], rsem, nbr[link]).start()
      maybe.extend(job[3] for job in jobs)

    def decode(jobs):
      wide = [dense_wide(src) for src, *_ in jobs]
      for src, n, to, _, _ in jobs:
        dense_decode(src, n, plain, to)
      @pl.when(functools.reduce(jnp.logical_or, wide))
      def _():
        for cond, (src, n, to, gaps, sem) in zip(wide, jobs):
          @pl.when(cond)
          def _():
            wait_recv(sem, gaps)
            dense_repair(src, n, gaps, plain, to)

    def wait_recv(rsem, ref):
      pltpu.make_async_copy(ref, ref, rsem).wait()

    def flag_of(word):
      return (word[0, 0] & 1) != 0
    def cast_a(r0, nr):
      a16[pl.ds(r0, nr), :] = a32[pl.ds(r0, nr), :].astype(BF16)
    def cast_b(c0, w):
      b16[:, pl.ds(c0, w)] = b32[:, pl.ds(c0, w)].astype(BF16)
    def part(role, s):
      return jnp.dot(a16[pl.ds(role * BLK + s * G, G), :], b16[...], preferred_element_type=F32)
    def stacked(v, r0):
      return [(v[r:r + 8, c:c + 128], v[r + 8:r + 16, c:c + 128]) for r in range(r0, r0 + Q, 16) for c in range(0, v.shape[1], 128)]
    def tiles(v, r0):
      return [(v[r:r + 8, c:c + 128], v[r:r + 8, c + 128:c + 256]) for r in range(r0, r0 + Q, 8) for c in range(0, N, 256)]
    def plus(ts, ws):
      return [(a + x, b + y) for (a, b), (x, y) in zip(ts, map(from_word, ws))]
    nkept = [0]
    def encode(ts, dst, at):
      mx = functools.reduce(jnp.maximum, [jnp.maximum(jnp.abs(a), jnp.abs(b)) for a, b in ts])
      ws, wide = dense_encode([to_word(a, b) for a, b in ts], mx, dst, at)
      k0 = nkept[0]
      nkept[0] += len(ws)
      for i, w in enumerate(ws):
        kept[k0 + i] = w
      return wide, k0, len(ws)
    def words(role, s, part):
      return cbuf.at[role, s, pl.ds(SPLIT[part], SPLIT[part + 1] - SPLIT[part])]
    def spill(role, s, part=None):
      lo, hi = (0, EXTRA // 2, EXTRA)[part or 0], (EXTRA // 2, EXTRA, EXTRA)[2 if part is None else part]
      return cbuf.at[role, s, pl.ds(MSG + lo, hi - lo)]
    def expand(role, s, chip, wait_extra, wait_late=lambda: None):
      def put(q, w):
        out_words[(2 * chip + s) * W + q] = w
      sparse_decode(cbuf.at[role, s], tmp, put, wait_extra, wait_late)

    @functools.partial(pl.run_scoped, lsem=pltpu.SemaphoreType.DMA((nload,)), rsem=pltpu.SemaphoreType.DMA((9,)), ssem=pltpu.SemaphoreType.DMA, osem=pltpu.SemaphoreType.DMA,
                       esem=pltpu.SemaphoreType.DMA((5,)), gsem=pltpu.SemaphoreType.DMA((2, NP + 4)))
    def _(lsem, rsem, ssem, osem, esem, gsem):
      sems.update(s=ssem, o=osem)
      R1, RU, G0, G1F, G1R, D0 = 0, 1, 5, 6, 7, 8
      for j in range(NFLAG):
        flags[j] = 0
      nl = [0]
      def load(src, dst):
        c = pltpu.make_async_copy(src, dst, lsem.at[nl[0]]); nl[0] += 1
        c.start()
        return c
      def load_a(role, r0, nr):
        return load(a_hbm.at[pl.ds(owner[role] * BLK + r0, nr)], a32.at[pl.ds(role * BLK + r0, nr)])
      loads = {}
      bar = pltpu.get_barrier_semaphore()
      for i, p in enumerate(plan):
        if p[0] == "a":
          loads[i] = load_a(DG, G * p[1], G)
        elif p[0] == "b":
          loads[i] = load(b_hbm.at[:, pl.ds(p[1], p[2])], b32.at[:, pl.ds(p[1], p[2])])
        if i == 1:
          for n in nbr:
            pl.semaphore_signal(bar, 1, device_id=(n,), device_id_type=MESH)
      for s in range(2):
        for role in (YP, XP):
          loads[role, s] = load_a(role, s * G, G)
      loads[ME, 0] = load_a(ME, 0, BLK)

      k = 0
      gaps1 = []
      for i, p in enumerate(plan):
        if p[0] == "a":
          with sc(f"wa{p[1]}"): loads[i].wait()
          cast_a(DG * BLK + p[1] * G, G)
        elif p[0] == "b":
          with sc(f"wb{p[1]}"): loads[i].wait()
          cast_b(p[1], p[2])
        else:
          _, q0, q1, c0, w, packed = p
          n, ln, at, to, at_gap = layout[k]
          v = jnp.dot(a16[pl.ds(DG * BLK + q0 * G, (q1 - q0) * G), :], b16[:, pl.ds(c0, w)], preferred_element_type=F32)
          enc = []
          for h in range(2):
            ts = [t for s in range(q1 - q0) for t in stacked(v, s * G + h * Q)]
            if packed:
              enc.append(encode(ts, s1.at[h], at + at_gap))
            else:
              for j, t in enumerate(ts):
                s1[h, at + at_gap + j] = to_word(*t)
          if k == 0:
            with sc("bar"): pl.semaphore_wait(bar, 2)
          with sc(f"s1_{i}"):
            for h in range(2):
              remote(lambda h=h, at=at, ln=ln, g=at_gap: (s1.at[h, pl.ds(at + g, ln)], r1.at[h, pl.ds(at, ln)]), h, rsem.at[R1])
          for h, e in enumerate(enc):
            gaps1.append(e + (lambda h=h, at=at, ln=ln, g=at_gap, n=n: (s1.at[h, pl.ds(at + g + ln, gap_len(n))], g1.at[h, pl.ds(g, gap_len(n))]),
                              h, gsem.at[h, k]))
          k += 1

      gaps2 = []
      def send_units(s, kind, enc):
        with sc(f"s{2 + kind}_{s}"):
          for link in range(2):
            remote(lambda link=link: (su.at[s, kind, link, pl.ds(0, LU)], ru.at[s, kind, link]), link, rsem.at[RU + 2 * s + kind])
        for link in range(2):
          gaps2.append(enc[link] + (lambda link=link: (su.at[s, kind, link, pl.ds(LU, GU)], gu.at[s, kind, link]), link, gsem.at[link, NP + 2 * s + kind]))
      def direct(s):
        for link in range(2):
          with sc(f"wn{s}{link}"): loads[YP + link, s].wait()
          for kind in range(2):
            a16[pl.ds(BLK * (1 + s) + kind * G + link * Q, Q), :] = a32[pl.ds((YP + link) * BLK + s * G + (kind ^ link) * Q, Q), :].astype(BF16)
        v = part(1 + s, 0)
        return [encode(tiles(v, link * Q), su.at[s, 0, link], 0) for link in range(2)]
      def stash(to, v):
        for j, (a, b) in enumerate(tiles(v, 0) + tiles(v, Q)):
          acc[to, j, 0] = a
          acc[to, j, 1] = b
      def relay(s):
        enc = []
        for link in range(2):
          got = {}
          for r in range(Q // 16):
            for c in range(N // 128):
              packed, j = where[s, r, c]
              got[2 * r, c], got[2 * r + 1, c] = from_word(plain[(1 - link) * DEC1 + j] if packed else r1[1 - link, j])
          ts = [tuple(acc[2 + s, link * U + j, e] + got[j // 4, 2 * (j % 4) + e] for e in range(2)) for j in range(U)]
          enc.append(encode(ts, su.at[s, 1, link], 0))
        send_units(s, 1, enc)
      send_units(0, 0, direct(0))
      stash(2, part(1, 1))
      later = direct(1)
      send_gaps(gaps1)
      with sc("w1"): wait_recv(rsem.at[R1], r1)
      packed = [(h, k) + lay for h in range(2) for k, lay in enumerate(layout) if lay[0] != lay[1]]
      decode([(r1.at[h, pl.ds(at, ln)], n, h * DEC1 + to, g1.at[h, pl.ds(at_gap, gap_len(n))], gsem.at[h, k])
              for h, k, n, ln, at, to, at_gap in packed])
      relay(0)
      send_units(1, 0, later)
      stash(3, part(2, 1))
      relay(1)
      send_gaps(gaps2)

      loads[ME, 0].wait(); cast_a(ME * BLK, BLK)
      for s in range(2):
        stash(s, part(ME, s))

      nm = len(maybe)
      @pl.loop(0, 2)
      def _(s):
        def arrived(kind):
          with sc("w3"): wait_recv(rsem.at[RU + 2 * s + kind], ru.at[s, kind])
          decode([(ru.at[s, kind, link], U, (kind ^ link) * U, gu.at[s, kind, link], gsem.at[link, NP + 2 * s + kind]) for link in range(2)])
        arrived(0)
        for q in range(W):
          (a, b), = plus([(acc[s, q, 0], acc[s, q, 1])], [plain[q]])
          acc[s, q, 0] = a
          acc[s, q, 1] = b
        arrived(1)
        def total(q):
          t, = plus([(acc[s, q, 0], acc[s, q, 1])], [plain[q]])
          z = jnp.concatenate(t, axis=0)
          zbuf[pl.ds(16 * q, 16)] = jnp.where(z < 0, 0.0, z)
          return to_word(zbuf[pl.ds(16 * q, 8, stride=2)], zbuf[pl.ds(16 * q + 1, 8, stride=2)])
        over = sparse_encode(total, tmp, cbuf.at[ME, s],
                             lambda q, w: out_words.__setitem__((2 * me + s) * W + q, w))
        flags[nm + s] = over.astype(I32)
        with sc("s4"):
          for first in (True, False):
            for link in range(2):
              p = 1 - link if first else link
              sem = rsem.at[jnp.where(s == 0, G0, G1F if first else G1R)]
              rcopy(words(ME, s, p), words(YP + link, s, p), ssem, sem, nbr[link]).start()
        @pl.when(over)
        def _():
          sparse_gaps(tmp, cbuf.at[ME, s])
          for link in range(2):
            rcopy(spill(ME, s), spill(YP + link, s), osem, esem.at[2 * s + link], nbr[link]).start()

      @pl.loop(0, 5)
      def _(i):
        s = jnp.where(i < 4, i // 2, 0)
        role = jnp.where(i < 4, YP + i % 2, DG)
        @pl.when(i == 0)
        def _():
          with sc("w4"): wait_recv(rsem.at[G0], cbuf.at[pl.ds(YP, 2), 0, pl.ds(0, MSG)])
          for link in range(2):
            part = pl.ds(17 * link, 17 - link)
            rcopy(cbuf.at[XP - link, 0, part], cbuf.at[DG, 0, part], ssem, rsem.at[D0], nbr[link]).start()
        @pl.when(i == 2)
        def _():
          with sc("w4"): wait_recv(rsem.at[G1F], cbuf.at[YP, 1, pl.ds(0, MSG)])
          for late in range(2):
            for link in range(2):
              part = pl.ds(16 * link + 13, 3 + link) if late else pl.ds(16 * link, 13)
              rcopy(cbuf.at[XP - link, 1, part], cbuf.at[DG, 1, part], ssem, fsem.at[late], nbr[link]).start()
          with sc("w5"): wait_recv(rsem.at[G1R], cbuf.at[YP, 1, pl.ds(0, MSG)])
        @pl.when(i == 4)
        def _():
          with sc("w6"): wait_recv(rsem.at[D0], cbuf.at[DG, 0, pl.ds(0, MSG)])
        def wait_extra(over):
          flags[nm + 2 + i] = over.astype(I32)
          pl.when(over & (i < 4))(lambda: wait_recv(esem.at[i], spill(role, s)))
          pl.when(over & (i == 4))(lambda: wait_recv(fsem.at[2], spill(DG, 0)))
          @pl.when(over & (i < 4))
          def _():
            part = pl.ds(MSG + (XP - role) * (EXTRA // 2), EXTRA // 2)
            rcopy(cbuf.at[role, s, part], cbuf.at[DG, s, part], osem, fsem.at[2 + s], jnp.where(role == XP, yp, xp)).start()
        chip = jnp.where(role == YP, yp, jnp.where(role == XP, xp, dg))
        with sc("dec"): expand(role, s, chip, wait_extra)

      with sc("wsend"):
        whole = lambda: (cbuf.at[ME, 0, pl.ds(0, MSG)],) * 2
        for refs in sends + [whole] * 6:
          rcopy(*refs(), ssem, fsem.at[0], me).wait_send()
        opt = list(enumerate(maybe))
        opt += [(nm + s, lambda: (spill(ME, 0),) * 2) for s in range(2) for _ in range(2)]
        opt += [(nm + 2 + i, lambda i=i: (spill(ME, 0, 1 - i % 2),) * 2) for i in range(4)]
        @pl.when(functools.reduce(jnp.bitwise_or, [flags[j] for j in range(NFLAG)]) != 0)
        def _():
          for j, refs in opt:
            @pl.when(flags[j] != 0)
            def _():
              rcopy(*refs(), osem, fsem.at[0], me).wait_send()

    with sc("w7"): wait_recv(fsem.at[0], cbuf.at[DG, 1, pl.ds(0, len(EARLY_AT))])
    def wait_extra(over):
      pl.when(over)(lambda: wait_recv(fsem.at[3], spill(DG, 1)))
    def wait_late():
      with sc("w8"): wait_recv(fsem.at[1], cbuf.at[DG, 1, pl.ds(0, len(LATE_AT))])
    expand(DG, 1, dg, wait_extra, wait_late)

  def f(A, B):
    wbuf = lambda *s: pltpu.VMEM(s + VREG, I32)
    tiled = pl.pallas_call(
        body,
        out_shape=jax.ShapeDtypeStruct((M * N // 2048, 16, 128), BF16),
        in_specs=[pl.BlockSpec(memory_space=pltpu.HBM)] * 2,
        out_specs=pl.BlockSpec(memory_space=pltpu.VMEM),
        scratch_shapes=[
            pltpu.VMEM((M, K), F32), pltpu.VMEM((K, N), F32), pltpu.VMEM((M, K), BF16), pltpu.VMEM((K, N), BF16),
            wbuf(2, LEN1 + GAP1), wbuf(2, LEN1), wbuf(2, GAP1), wbuf(max(2 * DEC1, W)),
            wbuf(2, 2, 2, LU + GU), wbuf(2, 2, 2, LU), wbuf(2, 2, 2, GU), wbuf(2 * DEC1 + 8 * U),
            pltpu.VMEM((4, W, 2) + VREG, F32), pltpu.VMEM((16 * W, 128), F32),
            wbuf(4, 2, MSG + EXTRA), wbuf(TMP),
            pltpu.SMEM((NFLAG,), I32),
            pltpu.SemaphoreType.DMA((4,)),
        ],
        compiler_params=pltpu.CompilerParams(collective_id=0, vmem_limit_bytes=48 * 2**20, **cp),
    )(A, B)
    return tiled.reshape(M // 8, N // 128, 8, 128).transpose(0, 2, 1, 3).reshape(M, N)
  return f


_kernel = make()


def pallas_dist_matmul_relu_kshard_i_m1024_n1024_k512_kernel(A: jax.Array, B: jax.Array):
  return _kernel(A, B)
```

```python
import functools

import jax
import jax.numpy as jnp
from jax import lax
from jax.experimental import pallas as pl
from jax.experimental.pallas import tpu as pltpu

F32, BF16, I32 = jnp.float32, jnp.bfloat16, jnp.int32
VREG = (8, 128)
srl = lax.shift_right_logical


def _i32(c):
  c &= 0xFFFFFFFF
  return c - (1 << 32) if c >> 31 else c


ONES = 0x00010001
SIGNS = _i32(0x80008000)
GAP = 0x78007800
WIDE = 0x70007000
MID = 0x08000800
LOW = 0x07FF07FF
HI = _i32(0xFFFF0000)
TOP = _i32(0x80000000)


def shift(x, n):
  return x << n if n > 0 else srl(x, -n) if n < 0 else x


def or_all(xs):
  return functools.reduce(lambda a, b: a | b, xs)


def pack_lo(a, b):
  return (a & 0xFFFF) | (b << 16)


def to_word(a, b):
  both = pltpu.bitcast(jnp.concatenate([a, b], axis=1).astype(BF16).astype(F32), I32)
  return srl(both[:, :128], 16) | both[:, 128:]


def from_word(w):
  return pltpu.bitcast(w << 16, F32), pltpu.bitcast(w & HI, F32)


def gap_len(n):
  return -(-n // 4)


def gap_words(ws):
  return [or_all([shift(w & GAP, 4 * j - 11) for j, w in enumerate(ws[k:k + 4])])
          for k in range(0, len(ws), 4)]


def gap_bits(ref, at, i):
  return shift(ref[at + i // 4], 11 - 4 * (i % 4)) & GAP


def mid_planes(ws):
  return [or_all([shift(w & MID, j - 11) for j, w in enumerate(ws[k:k + 16])])
          for k in range(0, len(ws), 16)]


def mid_bit(planes, i):
  return shift(planes[i // 16], 11 - i % 16) & MID


def dense_len(n):
  return 1 + 3 * n // 4


def dense_encode(ws, largest, dst, at):
  x = 3 * len(ws) // 4
  head = (srl(to_word(largest, largest), 7) - 31) & 0xFF
  base = head * (ONES << 7)
  ws = [w - base for w in ws]
  left = or_all(ws) & WIDE
  for k, z in enumerate(mid_planes(ws)):
    z = ~z
    for e in range(2):
      low = z & -z
      head = head | (lax.clz(low) << (8 + 12 * k + 6 * e))
      z = z ^ low
    left = left | z
  dst[at] = head | jnp.where(left != 0, 63 << 8, 0)
  for d, w in enumerate(ws[x:]):
    w = (w & LOW) | (srl(w, 4) & MID)
    for i in range(3):
      dst[at + 1 + 3 * d + i] = (ws[3 * d + i] & ~GAP) | ((w << (11 - 4 * i)) & GAP)
  return ws, jnp.where(left != 0, 1.0, 0.0)


def dense_has_gaps(src):
  return jnp.max(jnp.where((src[0] & (63 << 8)) == 63 << 8, 1.0, 0.0)) > 0


def dense_planes(src, n):
  planes = []
  for k in range(n // 16):
    at = [srl(src[0], 8 + 12 * k + 6 * e) for e in range(2)]
    planes.append(~or_all([srl(jnp.where((a & 32) != 0, 0, TOP), a & 31) for a in at]))
  return planes


def dense_decode(src, n, which, dst, to):
  x = 3 * n // 4
  base = (src[0] & 0xFF) * (ONES << 7)
  planes = dense_planes(src, n)
  for i in which:
    if i < x:
      w = src[1 + i] & ~GAP
    else:
      w = or_all([srl(src[1 + 3 * (i - x) + j] & GAP, 11 - 4 * j) for j in range(3)])
      w = (w & LOW) | ((w & MID) << 4)
    dst[to + i] = (w | mid_bit(planes, i)) + base


def dense_repair(src, n, which, gaps, dst, to):
  planes = dense_planes(src, n)
  for i in which:
    dst[to + i] = dst[to + i] - mid_bit(planes, i) + gap_bits(gaps, 0, i)


W = 64
C = 82
NV = C // 2
META = NV
MSG = 33
REST = 24
EXTRA = REST + gap_len(NV) + 1
T_W, T_T, T_D, T_X, TMP = 0, W, 2 * W, 3 * W, 5 * W
PAIRS = ((0, 3), (1, 2), (4, 7), (5, 6))
CUT_AT = 16
LATE_AT = list(range(13, 16)) + list(range(29, 33))
EARLY_AT = [i for i in range(MSG) if i not in LATE_AT]
FLAG_AT = EARLY_AT[:4]
EARLY_V = [5 * r + i for pair in PAIRS[:3] for r in pair for i in range(5)] + [NV - 1, META]
LATE_V = [5 * r + i for r in PAIRS[3] for i in range(5)]


def _spread(vs, ats):
  return {v: [(ats[2 * k], 11, ~LOW), (ats[2 * k + 1], 6, ~LOW),
              (ats[2 * len(vs) + k // 5], 1 + k % 5, _i32(MID << (k % 5)))]
          for k, v in enumerate(vs)}


HOME = dict(list(zip(EARLY_V[:22], EARLY_AT[4:])) + list(zip(LATE_V[:7], LATE_AT)))
SPREAD = {**_spread(EARLY_V[22:], EARLY_AT[4:]), **_spread(LATE_V[7:], LATE_AT)}


def partner(x):
  return pltpu.roll(x, 4, 0)


def pair_total(cnt):
  n = (cnt & 0xFFFF) + srl(cnt, 16)
  return n + partner(n)


def slot_at(j):
  return (NV - 1, j % 2) if j >= 80 else (5 * (j % 8) + j // 16, (j // 8) % 2)


def rest_at(p):
  m = p // 8 - (11 if p % 8 < 2 else 10)
  return 3 * (p % 8) + m // 2, m % 2


def sparse_encode(word, tmp, dst, midway):
  cnt = largest = jnp.zeros(VREG, I32)
  for q in range(W):
    w = word(q) & ~SIGNS
    largest = jnp.maximum(largest, jnp.maximum(w, w << 16))
    t = (w + ~SIGNS) & SIGNS
    tmp[T_W + q] = w
    tmp[T_T + q] = t
    tmp[T_D + q] = q * ONES - cnt
    cnt = cnt + srl(t, 15)
  for k, at in enumerate(FLAG_AT):
    dst[at] = or_all([shift(tmp[T_T + 16 * k + j], -j) for j in range(16)])
  z_lo = W - (cnt & 0xFFFF)
  b = (srl(largest, 23) - 31) & 0xFF
  base = b * (ONES << 7)

  stay = [{}, {}, {}]

  def push(k, i, x):
    if k == 3:
      tmp[T_X + i] = x
      return
    s = 1 << k
    if i < s:
      stay[k][i] = x
      return
    m = (x & s) != 0
    stay[k][i] = jnp.where(m, 0, x)
    push(k + 1, i - s, jnp.where(m, x, stay[k].pop(i - s)))

  seen = small_cnt = jnp.zeros(VREG, I32)
  for q in range(W):
    t = tmp[T_T + q]
    w = (((tmp[T_W + q] | SIGNS) - base) ^ MID) & (t - srl(t, 15))
    tmp[T_W + q] = w
    seen = seen | w
    small_cnt = small_cnt + srl(w & MID, 11)
    push(0, q, pack_lo(tmp[T_D + q], w))
  full = pair_total(cnt) > 2 * C
  more = full | (pair_total(small_cnt) > 2) | ((seen & WIDE) != 0)
  more = jnp.max(jnp.max(jnp.where(more, 1.0, 0.0), axis=1, keepdims=True), axis=0, keepdims=True)
  for q in range(W):
    push(0, W + q, (tmp[T_W + q] & HI) | (srl(tmp[T_D + q], 16) + z_lo))
  for k in range(3):
    for i in sorted(stay[k]):
      push(k + 1, i, stay[k].pop(i))
  midway()

  share = jnp.where(full, 0, -1)
  pack = lambda lo, hi: srl(lo, 16) | (hi & HI)
  last = {}
  for pair in PAIRS:
    x = {}
    for r in pair:
      v = [tmp[T_X + r + 8 * m] for m in range(16)]
      for s in (1, 2, 4, 8):
        mv = [None] * s + [(v[m] & (8 * s)) != 0 for m in range(s, 16)]
        st = [v[m] if mv[m] is None else jnp.where(mv[m], 0, v[m]) for m in range(16)]
        v = [jnp.where(mv[m + s], v[m + s], st[m]) if m + s < 16 else st[m] for m in range(16)]
      for m in range(16):
        x[r + 8 * m] = v[m]

    def slot(j):
      o = 2 * C - 1 - j
      return x[j] | (partner(x[o]) & share) if o < 2 * W else x[j]

    for r in pair:
      for i in range(5):
        tmp[T_W + 5 * r + i] = pack(slot(r + 16 * i), slot(r + 16 * i + 8))
      for i in range(3):
        p = r + (88 if r < 2 else 80) + 16 * i
        dst[MSG + 3 * r + i] = pack(x[p], x[p + 8]) if p + 8 < 2 * W else srl(x[p], 16)
      if r < 2:
        last[r] = slot(80 + r)
  tmp[T_W + NV - 1] = pack(last[0], last[1])

  z = mid_planes([tmp[T_W + i] for i in range(NV)])
  small = []
  for _ in range(2):
    m0, m01 = z[0] != 0, (z[0] | z[1]) != 0
    cur = jnp.where(m0, z[0], jnp.where(m01, z[1], z[2]))
    low = cur & -cur
    small.append(lax.clz(low) + jnp.where(m0, 0, jnp.where(m01, 32, 64)))
    z = [z[0] ^ jnp.where(m0, low, 0), z[1] ^ jnp.where(m0, 0, jnp.where(m01, low, 0)),
         z[2] ^ jnp.where(m01, 0, low)]
  more = jnp.where(jnp.broadcast_to(more, VREG) > 0, 127, 0)
  meta = b | ((small[0] | more) << 8) | (small[1] << 15)
  tmp[T_W + META] = (meta & 0x7FF) | (srl(meta, 11) << 16)
  pieces = {}
  for v, where in SPREAD.items():
    for at, sh, mask in where:
      pieces.setdefault(at, []).append((tmp[T_W + v] << sh) & mask)
  for v, at in HOME.items():
    dst[at] = or_all([tmp[T_W + v] & LOW] + pieces[at])
  return more[0, 0] > 0


def sparse_gaps(tmp, dst):
  for k, g in enumerate(gap_words([tmp[T_W + i] for i in range(NV)])):
    dst[MSG + REST + k] = g
  dst[MSG + EXTRA - 1] = jnp.zeros(VREG, I32)


def sparse_decode(src, tmp, put, wait_extra, wait_late):
  def gather(v):
    return or_all([srl(src[at] & mask, sh) for at, sh, mask in SPREAD[v]])

  w = gather(META)
  meta = (w & 0x7FF) | (srl(w, 16) << 11)
  small = [srl(meta, 8) & 127, srl(meta, 15)]
  cnt = jnp.zeros(VREG, I32)
  for q in range(W):
    t = shift(src[FLAG_AT[q // 16]], q % 16) & SIGNS
    g = srl(t, 15)
    tmp[T_T + q] = t - g
    tmp[T_D + q] = q * ONES - cnt
    cnt = cnt + g
  wait_extra(small[0][0, 0] == 127)
  more, full = small[0] == 127, pair_total(cnt) > 2 * C
  z_lo = (W - (cnt & 0xFFFF)) << 16
  base = (meta & 0xFF) * (ONES << 7)
  planes = [or_all([srl(jnp.where(srl(a, 5) == k, TOP, 0), a & 31) for a in small]) for k in range(3)]

  def unpack(vs):
    for v in vs:
      w = gather(v) if v in SPREAD else src[HOME[v]] & LOW
      tmp[T_W + v] = w | jnp.where(more, gap_bits(src, MSG + REST, v), mid_bit(planes, v))

  def dist(p):
    return (tmp[T_D + p], 0) if p < W else (tmp[T_D + p - W] + z_lo, 16)

  def half(w, h):
    return srl(w, 16) if h else w

  def start(p):
    if p < C:
      i, h = slot_at(p)
      return half(tmp[T_W + i], h)
    i, h = slot_at(2 * C - 1 - p)
    j, k = rest_at(p)
    return jnp.where(full, half(src[MSG + j], k), half(partner(tmp[T_W + i]), h))

  unpack(EARLY_V[:-1])
  for pair in PAIRS:
    if pair == PAIRS[-1]:
      wait_late()
      unpack(LATE_V)
    for r in pair:
      v = [start(r + 8 * m) for m in range(16)]
      d = [None] + [dist(r + 8 * m) for m in range(1, 16)]
      for s in (8, 4, 2, 1):
        v = [v[m] if m < s else jnp.where((d[m][0] & ((8 * s) << d[m][1])) != 0, v[m - s], v[m])
             for m in range(16)]
      for m in range(16):
        tmp[T_X + r + 8 * m] = v[m]
  behind = [[{}, {}, {}], [{}, {}, {}]]

  def finish(h, p):
    x = tmp[T_X + p]
    d, off = dist(p)
    for k in (2, 1, 0):
      s = 1 << k
      behind[h][k][p] = x
      if p - s in behind[h][k]:
        x = jnp.where((d & (s << off)) != 0, behind[h][k].pop(p - s), x)
    return x

  for p in range(W - 7, W):
    finish(1, p)
  for q in range(W):
    put(q, ((pack_lo(finish(0, q), finish(1, W + q)) ^ MID) + base) & tmp[T_T + q])


M, N, K = 1024, 1024, 512
BLK = M // 4
G = BLK // 2
Q = G // 2
U = Q * N // 2048
LU, GU = dense_len(U), gap_len(U)
DG, YP, XP, ME = range(4)
HEAD = 3
MESH = pl.DeviceIdType.MESH

PLAN = (
    ("b", 0, 128), ("a", 0), ("p", 0, 1, 0, 128, False), ("a", 1), ("p", 1, 2, 0, 128, False),
    ("b", 128, 128), ("p", 0, 1, 128, 128, False), ("p", 1, 2, 128, 128, False),
    ("b", 256, 128), ("p", 0, 2, 256, 128, False), ("b", 384, 128), ("p", 0, 2, 384, 128, False),
    ("b", 512, 256), ("p", 0, 2, 512, 256, True), ("b", 768, 256), ("p", 0, 2, 768, 256, True),
)


def _lay_out():
  pieces, place, at, to, at_gap = [], {}, 0, 0, 0
  for p in PLAN:
    if p[0] == "p":
      _, s0, s1, c0, w, encoded = p
      keys = [(s, r, c) for s in range(s0, s1) for r in range(Q // 16)
              for c in range(c0 // 128, (c0 + w) // 128)]
      n = len(keys)
      place.update({key: (encoded, (to if encoded else at) + i) for i, key in enumerate(keys)})
      ln = dense_len(n) if encoded else n
      pieces.append((n, ln, at, to, at_gap))
      at += ln
      if encoded:
        to, at_gap = to + n, at_gap + gap_len(n)
  return pieces, place, at, to, at_gap


PIECES, PLACE, LEN1, DEC1, GAP1 = _lay_out()
ENCODED = [(h, k) + p for h in range(2) for k, p in enumerate(PIECES) if p[0] != p[1]]
NLOAD = sum(p[0] != "p" for p in PLAN) + 5
NFLAG = len(ENCODED) + 8 + 2 + 5


def _body(a_hbm, b_hbm, out, a32, b32, a16, b16, s1, r1, g1, plain, su, ru, gu, kept, acc,
          cbuf, tmp, flags, fsem):
  me = lax.axis_index("i")
  yp, xp, dg = me ^ 1, 3 - me, me ^ 2
  nbr = (yp, xp)
  owner = (dg, yp, xp, me)

  def rcopy(src, dst, send_sem, recv_sem, dev):
    return pltpu.make_async_remote_copy(src, dst, send_sem, recv_sem, device_id=(dev,), device_id_type=MESH)

  def wait_recv(sem, ref):
    pltpu.make_async_copy(ref, ref, sem).wait()

  def spill(role, s):
    return cbuf.at[role, s, pl.ds(MSG, EXTRA)]

  def expand(role, s, chip, wait_extra, wait_late=lambda: None):
    def put(q, w):
      out[(2 * chip + s) * W + q] = pltpu.bitcast(w, BF16)
    sparse_decode(cbuf.at[role, s], tmp, put, wait_extra, wait_late)

  def cast_a(r0, nr):
    a16[pl.ds(r0, nr), :] = a32[pl.ds(r0, nr), :].astype(BF16)

  def product(r0):
    return jnp.dot(a16[pl.ds(r0, G), :], b16[...], preferred_element_type=F32)

  def stacked(v, r0):
    return [(v[r:r + 8, c:c + 128], v[r + 8:r + 16, c:c + 128])
            for r in range(r0, r0 + Q, 16) for c in range(0, v.shape[1], 128)]

  def tiles(v, r0):
    return [(v[r:r + 8, c:c + 128], v[r:r + 8, c + 128:c + 256])
            for r in range(r0, r0 + Q, 8) for c in range(0, N, 256)]

  def stash(to, v):
    for j, (a, b) in enumerate(tiles(v, 0) + tiles(v, Q)):
      acc[to, j, 0] = a
      acc[to, j, 1] = b

  nkept = [0]

  def encode(ts, dst, at):
    largest = functools.reduce(jnp.maximum, [jnp.maximum(jnp.abs(a), jnp.abs(b)) for a, b in ts])
    ws, wide = dense_encode([to_word(a, b) for a, b in ts], largest, dst, at)
    k0 = nkept[0]
    nkept[0] += len(ws)
    for i, w in enumerate(ws):
      kept[k0 + i] = w
    return wide, k0, len(ws)

  def decode(jobs, wait=True):
    has_gaps = [dense_has_gaps(job[0]) for job in jobs]
    for src, n, which, to, _, _ in jobs:
      dense_decode(src, n, which, plain, to)

    @pl.when(functools.reduce(jnp.logical_or, has_gaps))
    def _():
      for cond, (src, n, which, to, gaps, sem) in zip(has_gaps, jobs):
        @pl.when(cond)
        def _():
          if wait:
            wait_recv(sem, gaps)
          dense_repair(src, n, which, gaps, plain, to)

  dma = pltpu.SemaphoreType.DMA

  @functools.partial(pl.run_scoped, lsem=dma((NLOAD,)), rsem=dma((10,)), ssem=dma(()), osem=dma(()),
                     esem=dma((4,)), gsem=dma((2, len(PIECES) + 4)))
  def _(lsem, rsem, ssem, osem, esem, gsem):
    R1, RU, G0H, G0, G1F, G1R, D0 = 0, 1, 5, 6, 7, 8, 9
    for j in range(NFLAG):
      flags[j] = 0
    sends, maybe, loads = [], [], {}

    def send(src, dst, link, sem):
      sends.append(rcopy(src, dst, ssem, sem, nbr[link]))
      sends[-1].start()

    def send_gaps(jobs):
      @pl.when(jnp.max(functools.reduce(jnp.maximum, [job[0] for job in jobs])) > 0)
      def _():
        for j, (wide, at, n, src, dst, link, sem) in enumerate(jobs):
          cond = jnp.max(wide) > 0
          flags[len(maybe) + j] = cond.astype(I32)

          @pl.when(cond)
          def _():
            for k, g in enumerate(gap_words([kept[at + i] for i in range(n)])):
              src[k] = g
            rcopy(src, dst, osem, sem, nbr[link]).start()
      maybe.extend(job[3] for job in jobs)

    def load(key, src, dst):
      loads[key] = pltpu.make_async_copy(src, dst, lsem.at[len(loads)])
      loads[key].start()

    def load_a(key, role, r0, nr):
      load(key, a_hbm.at[pl.ds(owner[role] * BLK + r0, nr)], a32.at[pl.ds(role * BLK + r0, nr)])

    barrier = pltpu.get_barrier_semaphore()
    for i, p in enumerate(PLAN):
      if p[0] == "a":
        load_a(i, DG, G * p[1], G)
      elif p[0] == "b":
        load(i, b_hbm.at[:, pl.ds(p[1], p[2])], b32.at[:, pl.ds(p[1], p[2])])
      if i == 1:
        for n in nbr:
          pl.semaphore_signal(barrier, 1, device_id=(n,), device_id_type=MESH)
    for s in range(2):
      for role in (YP, XP):
        load_a((role, s), role, s * G, G)
    load_a(ME * 100, ME, 0, BLK)

    k = 0
    gaps1 = []
    for i, p in enumerate(PLAN):
      if p[0] == "a":
        loads[i].wait()
        cast_a(DG * BLK + p[1] * G, G)
      elif p[0] == "b":
        loads[i].wait()
        b16[:, pl.ds(p[1], p[2])] = b32[:, pl.ds(p[1], p[2])].astype(BF16)
      else:
        _, q0, q1, c0, w, encoded = p
        n, ln, at, _, at_gap = PIECES[k]
        v = jnp.dot(a16[pl.ds(DG * BLK + q0 * G, (q1 - q0) * G), :], b16[:, pl.ds(c0, w)],
                    preferred_element_type=F32)
        for h in range(2):
          ts = [t for s in range(q1 - q0) for t in stacked(v, s * G + h * Q)]
          if encoded:
            gaps1.append(encode(ts, s1.at[h], at_gap + at) + (
                s1.at[h, pl.ds(at_gap + at + ln, gap_len(n))], g1.at[h, pl.ds(at_gap, gap_len(n))],
                h, gsem.at[h, k]))
          else:
            for j, t in enumerate(ts):
              s1[h, at_gap + at + j] = to_word(*t)
        if k == 0:
          pl.semaphore_wait(barrier, 2)
        for h in range(2):
          send(s1.at[h, pl.ds(at_gap + at, ln)], r1.at[h, pl.ds(at, ln)], h, rsem.at[R1])
        k += 1

    gaps2 = []

    def send_units(s, kind, enc):
      for link in range(2):
        send(su.at[s, kind, link, pl.ds(0, LU)], ru.at[s, kind, link], link, rsem.at[RU + 2 * s + kind])
        gaps2.append(enc[link] + (su.at[s, kind, link, pl.ds(LU, GU)], gu.at[s, kind, link],
                                  link, gsem.at[link, len(PIECES) + 2 * s + kind]))

    def direct(s):
      for link in range(2):
        loads[YP + link, s].wait()
        for kind in range(2):
          a16[pl.ds(BLK * (1 + s) + kind * G + link * Q, Q), :] = (
              a32[pl.ds((YP + link) * BLK + s * G + (kind ^ link) * Q, Q), :].astype(BF16))
      v = product(BLK * (1 + s))
      return [encode(tiles(v, link * Q), su.at[s, 0, link], 0) for link in range(2)]

    def relay(s):
      decode([(r1.at[h, pl.ds(at, ln)], n, range(s * n // 2, (s + 1) * n // 2), h * DEC1 + to,
               g1.at[h, pl.ds(at_gap, gap_len(n))], gsem.at[h, k])
              for h, k, n, ln, at, to, at_gap in ENCODED], wait=s == 0)
      enc = []
      for link in range(2):
        got = {}
        for r in range(Q // 16):
          for c in range(N // 128):
            encoded, j = PLACE[s, r, c]
            got[2 * r, c], got[2 * r + 1, c] = from_word(
                plain[(1 - link) * DEC1 + j] if encoded else r1[1 - link, j])
        ts = [tuple(acc[2 + s, link * U + j, e] + got[j // 4, 2 * (j % 4) + e] for e in range(2))
              for j in range(U)]
        enc.append(encode(ts, su.at[s, 1, link], 0))
      send_units(s, 1, enc)

    send_units(0, 0, direct(0))
    stash(2, product(BLK + G))
    later = direct(1)
    send_gaps(gaps1)
    wait_recv(rsem.at[R1], r1)
    relay(0)
    send_units(1, 0, later)
    stash(3, product(2 * BLK + G))
    relay(1)
    send_gaps(gaps2)

    loads[ME * 100].wait()
    cast_a(ME * BLK, BLK)
    for s in range(2):
      stash(s, product(ME * BLK + s * G))
    nm = len(maybe)

    @pl.loop(0, 2)
    def _(s):
      def arrived(kind):
        wait_recv(rsem.at[RU + 2 * s + kind], ru.at[s, kind])
        decode([(ru.at[s, kind, link], U, range(U), (kind ^ link) * U, gu.at[s, kind, link],
                 gsem.at[link, len(PIECES) + 2 * s + kind]) for link in range(2)])

      def plus(q):
        lo, hi = from_word(plain[q])
        return acc[s, q, 0] + lo, acc[s, q, 1] + hi

      arrived(0)
      for q in range(W):
        acc[s, q, 0], acc[s, q, 1] = plus(q)
      arrived(1)

      def word(q):
        z = jnp.concatenate(plus(q), axis=0)
        z = jnp.where(z < 0, 0.0, z).astype(BF16)
        out[(2 * me + s) * W + q] = z
        return pltpu.bitcast(z, I32)

      def midway():
        @pl.when(s == 1)
        def _():
          wait_recv(rsem.at[G0H], cbuf.at[pl.ds(YP, 2), 0, pl.ds(0, HEAD)])
          for link in range(2):
            part = pl.ds((MSG - HEAD) * link, HEAD)
            rcopy(cbuf.at[XP - link, 0, part], cbuf.at[DG, 0, part], ssem, rsem.at[D0], nbr[link]).start()

      more = sparse_encode(word, tmp, cbuf.at[ME, s], midway)
      flags[nm + s] = more.astype(I32)
      order = (((MSG - HEAD, HEAD), (CUT_AT, MSG - HEAD - CUT_AT), (0, CUT_AT)),
               ((0, HEAD), (HEAD, CUT_AT - HEAD), (CUT_AT, MSG - CUT_AT)))
      for j, (first, second) in enumerate(((G0H, G1F), (G0, G1F), (G0, G1R))):
        for link in range(2):
          part = pl.ds(*order[link][j])
          rcopy(cbuf.at[ME, s, part], cbuf.at[YP + link, s, part], ssem,
                rsem.at[jnp.where(s == 0, first, second)], nbr[link]).start()

      @pl.when(more)
      def _():
        sparse_gaps(tmp, cbuf.at[ME, s])
        for link in range(2):
          rcopy(spill(ME, s), spill(YP + link, s), osem, esem.at[2 * s + link], nbr[link]).start()

    @pl.loop(0, 5)
    def _(i):
      s = jnp.where(i < 4, i // 2, 0)
      role = jnp.where(i < 4, YP + i % 2, DG)

      @pl.when(i == 0)
      def _():
        wait_recv(rsem.at[G0], cbuf.at[pl.ds(YP, 2), 0, pl.ds(0, MSG - HEAD)])
        for link in range(2):
          part = pl.ds(17, MSG - HEAD - 17) if link else pl.ds(HEAD, 17 - HEAD)
          rcopy(cbuf.at[XP - link, 0, part], cbuf.at[DG, 0, part], ssem, rsem.at[D0], nbr[link]).start()

      @pl.when(i == 2)
      def _():
        wait_recv(rsem.at[G1F], cbuf.at[YP, 1, pl.ds(0, MSG)])
        for late in range(2):
          for link in range(2):
            part = pl.ds(CUT_AT * link + 13, 3 + link) if late else pl.ds(CUT_AT * link, 13)
            rcopy(cbuf.at[XP - link, 1, part], cbuf.at[DG, 1, part], ssem, fsem.at[late], nbr[link]).start()
        wait_recv(rsem.at[G1R], cbuf.at[YP, 1, pl.ds(0, MSG)])

      @pl.when(i == 4)
      def _():
        wait_recv(rsem.at[D0], cbuf.at[DG, 0, pl.ds(0, MSG)])

      def wait_extra(more):
        flags[nm + 2 + i] = more.astype(I32)
        pl.when(more & (i < 4))(lambda: wait_recv(esem.at[i], spill(role, s)))
        pl.when(more & (i == 4))(lambda: wait_recv(fsem.at[2], spill(DG, 0)))

        @pl.when(more & (i < 4))
        def _():
          part = pl.ds(MSG + (XP - role) * (EXTRA // 2), EXTRA // 2)
          rcopy(cbuf.at[role, s, part], cbuf.at[DG, s, part], osem, fsem.at[2 + s],
                jnp.where(role == XP, yp, xp)).start()

      expand(role, s, jnp.where(role == YP, yp, jnp.where(role == XP, xp, dg)), wait_extra)

    def wait_send(ref, sem):
      rcopy(ref, ref, sem, fsem.at[0], me).wait_send()

    for c in sends:
      c.wait_send()
    for _ in range(6):
      wait_send(cbuf.at[ME, 0, pl.ds(0, MSG)], ssem)

    @pl.when(functools.reduce(jnp.bitwise_or, [flags[j] for j in range(NFLAG)]) != 0)
    def _():
      optional = list(enumerate(maybe))
      optional += [(nm + s, spill(ME, s)) for s in range(2) for _ in range(2)]
      optional += [(nm + 2 + i, cbuf.at[ME, 0, pl.ds(MSG, EXTRA // 2)]) for i in range(4)]
      for j, ref in optional:
        pl.when(flags[j] != 0)(functools.partial(wait_send, ref, osem))

  wait_recv(fsem.at[0], cbuf.at[DG, 1, pl.ds(0, len(EARLY_AT))])
  expand(DG, 1, dg,
         lambda more: pl.when(more)(lambda: wait_recv(fsem.at[3], spill(DG, 1))),
         lambda: wait_recv(fsem.at[1], cbuf.at[DG, 1, pl.ds(0, len(LATE_AT))]))


def pallas_dist_matmul_relu_kshard_i_m1024_n1024_k512_kernel(A: jax.Array, B: jax.Array):
  words = lambda *shape: pltpu.VMEM(shape + VREG, I32)
  tiled = pl.pallas_call(
      _body,
      out_shape=jax.ShapeDtypeStruct((M * N // 2048, 16, 128), BF16),
      in_specs=[pl.BlockSpec(memory_space=pltpu.HBM)] * 2,
      out_specs=pl.BlockSpec(memory_space=pltpu.VMEM),
      scratch_shapes=[
          pltpu.VMEM((M, K), F32), pltpu.VMEM((K, N), F32),
          pltpu.VMEM((M, K), BF16), pltpu.VMEM((K, N), BF16),
          words(2, LEN1 + GAP1), words(2, LEN1), words(2, GAP1),
          words(max(2 * DEC1, W)),
          words(2, 2, 2, LU + GU), words(2, 2, 2, LU), words(2, 2, 2, GU),
          words(2 * DEC1 + 8 * U),
          pltpu.VMEM((4, W, 2) + VREG, F32),
          words(4, 2, MSG + EXTRA), words(TMP),
          pltpu.SMEM((NFLAG,), I32),
          pltpu.SemaphoreType.DMA((4,)),
      ],
      compiler_params=pltpu.CompilerParams(collective_id=0, vmem_limit_bytes=48 * 2**20),
  )(A, B)
  return tiled.reshape(M // 8, N // 128, 8, 128).transpose(0, 2, 1, 3).reshape(M, N)
```
